```python
import numpy as np

kernel_name = "dist_matmul_mk_i_outk_m1024_n1024_k512"

def setup_inputs():
    A = np.random.randn(1024, 2048).astype(np.float32)
    B = np.random.randn(2048, 1024).astype(np.float32)
    return {"A": A, "B": B}

def reference(A: np.ndarray, B: np.ndarray) -> np.ndarray:
    return A @ B
```

```python
import jax
import jax.numpy as jnp
from jax import lax
from jax.experimental import pallas as pl
from jax.experimental.pallas import tpu as pltpu

M, K, N = 1024, 512, 1024
CH = 256
NB = N // 128
BF = jnp.bfloat16
F32 = jnp.float32

LO = 96
HI = CH - LO
F = HI - LO
NS = F // 16
NQ = NS * NB
_D = 10
Q = (NQ // 2, NQ // 2 - _D, NQ // 2, NQ // 2 + _D)

RG = (0, 16, 48, 80, 96, 128, 160, 192)
MID0 = 4 * LO
C0 = MID0 + F
OWN0 = C0 + 2 * HI

ORDER = ("B0 R0 R1 R2 R3 R4 R5 R6 B1 B2 B3 B4 B5 B6 B7 M C O").split()
PIECES = (
    (0, 1, 0, 1, (0, 1)),
    (1, 2, 0, 1, (1, 2)),
    (2, 3, 0, 1, (2, 3)),
    (3, 5, 0, 1, (3, 5)),
    (5, 6, 0, 1, (5, 6)),
    (6, 7, 0, 1, (6, 7)),
    (0, 4, 1, 2, (0, 1, 2, 4)),
    (4, 7, 1, 2, (4, 7)),
    (0, 4, 2, 3, (0, 4)),
    (0, 4, 3, 4, (0, 4)),
    (0, 4, 4, 6, (0, 4)),
    (0, 4, 6, 8, (0, 4)),
    "M",
    (4, 7, 2, 5, (4, 7)),
    (4, 7, 5, 8, (4, 7)),
)
PC = (("V", 0, 4), ("V", 4, 8), "own", ("F", 0, 6), ("F", 6, 8))

N_LOAD_SEMS = sum(2 if it[0] in "RC" else 1 for it in ORDER)
N_RDMA_SEMS = (2
               + 2 * sum(len(p[4]) - 1 for p in PIECES if p != "M")
               + 2 * sum(1 for p in PC if p != "own"))


def _body(a_hbm, b_hbm, o_ref, a32, b32, sv, rv, sm, rm, scv, rcv, scf, rcf, pc,
          lsem, ssem, rsem):
    me = lax.axis_index("i")
    p1 = me ^ 1
    p2 = 3 - me
    dg = me ^ 2
    nbr = (p1, p2)

    def a_items(item):
        if item[0] == "R":
            g = int(item[1:])
            v0, v1 = RG[g], RG[g + 1]
            n = v1 - v0
            if v0 < LO:
                return [(dg, v0, n, 2 * v0), (dg, HI + v0, n, 2 * v0 + n)]
            return [(p1, v0 - LO, n, 2 * v0), (p2, HI + v0 - LO, n, 2 * v0 + n)]
        if item == "M":
            return [(dg, LO, F, MID0)]
        if item == "C":
            return [(p1, LO, HI, C0), (p2, 0, HI, C0 + HI)]
        return [(me, 0, CH, OWN0)]

    loads = {}
    k = 0
    for item in ORDER:
        cps = []
        if item[0] == "B":
            cb = int(item[1:])
            cps.append(pltpu.make_async_copy(
                b_hbm.at[:, pl.ds(cb * 128, 128)], b32.at[cb], lsem.at[k]))
            k += 1
        else:
            for (c, r0, n, d0) in a_items(item):
                src = pl.multiple_of(c * CH + r0, 16)
                cps.append(pltpu.make_async_copy(
                    a_hbm.at[pl.ds(src, n), :], a32.at[pl.ds(d0, n), :], lsem.at[k]))
                k += 1
        loads[item] = cps

    bar = pltpu.get_barrier_semaphore()
    for i, item in enumerate(ORDER):
        for cp in loads[item]:
            cp.start()
        if i == 0:
            for nb in nbr:
                pl.semaphore_signal(bar, inc=1, device_id=(nb,),
                                    device_id_type=pl.DeviceIdType.MESH)

    def q_of(x):
        r = jnp.int32(Q[0])
        for pos in range(1, 4):
            r = jnp.where(x == pos, jnp.int32(Q[pos]), r)
        return r

    q_p1, q_p2 = q_of(p1), q_of(p2)

    loaded = set()

    def need(items):
        for it in sorted(items, key=ORDER.index):
            if it not in loaded:
                loaded.add(it)
                for cp in loads[it]:
                    cp.wait()

    def lhs(r0, n):
        return a32[pl.ds(r0, n), :].astype(BF)

    def mm(x, cb):
        return jnp.dot(x, b32[cb].astype(BF), preferred_element_type=F32)

    next_sem = [2]

    def rdma(src, dst, link, kk=None):
        if kk is None:
            kk = next_sem[0]
            next_sem[0] += 1
        return pltpu.make_async_remote_copy(
            src_ref=src, dst_ref=dst, send_sem=ssem.at[kk], recv_sem=rsem.at[kk],
            device_id=(nbr[link],), device_id_type=pl.DeviceIdType.MESH)

    def mid_copy(sender_pos, link):
        lo, hi = (0, Q[sender_pos]) if link == 0 else (Q[sender_pos], NQ)
        return rdma(sm.at[pl.ds(lo, hi - lo)], rm.at[link, pl.ds(lo, hi - lo)], link, link)

    sends = []
    recv_a = []
    recv_b = []
    first = True
    for p in PIECES:
        if p == "M":
            need(["M"] + [f"B{c}" for c in range(NB)])
            x = lhs(MID0, F)
            for cb in range(NB):
                res = mm(x, cb).astype(BF)
                for s in range(NS):
                    sm[s * NB + cb] = res[16 * s:16 * s + 16]
            for pos in range(4):
                @pl.when(me == pos)
                def _(pos=pos):
                    for link in range(2):
                        mid_copy(pos, link).start()
            continue
        g0, g1, c0, c1, subs = p
        need([f"R{g}" for g in range(g0, g1)] + [f"B{c}" for c in range(c0, c1)])
        v0, v1 = RG[g0], RG[g1]
        x = lhs(2 * v0, 2 * (v1 - v0))
        ress = [mm(x, cb).astype(BF) for cb in range(c0, c1)]
        for h0, h1 in zip(subs[:-1], subs[1:]):
            for cb in range(c0, c1):
                res = ress[cb - c0]
                for g in range(h0, h1):
                    w0, w1 = RG[g], RG[g + 1]
                    n = w1 - w0
                    off = 2 * (w0 - v0)
                    sv[0, cb, w0:w1, :] = res[off:off + n]
                    sv[1, cb, w0:w1, :] = res[off + n:off + 2 * n]
            u0, u1 = RG[h0], RG[h1]
            cps = [rdma(sv.at[link, pl.ds(c0, c1 - c0), pl.ds(u0, u1 - u0), :],
                        rv.at[link, pl.ds(c0, c1 - c0), pl.ds(u0, u1 - u0), :], link)
                   for link in range(2)]
            if first:
                pl.semaphore_wait(bar, 2)
                first = False
            for cp in cps:
                cp.start()
            sends += cps
            if u0 < LO:
                recv_a.append((c0, c1, cps))
            else:
                recv_b += cps

    need(["C"])
    x = lhs(C0, 2 * HI)
    for cb in range(NB):
        pc[cb] = mm(x, cb)

    a_waited = set()
    mid_waited = False
    recv_c = []
    for item in PC:
        if item == "own":
            need(["O"])
            x = lhs(OWN0, CH)
            for cb in range(NB):
                o_ref[:, cb * 128:(cb + 1) * 128] = mm(x, cb)
            continue
        part, c0, c1 = item
        if part == "V":
            for i, (a0, a1, cps) in enumerate(recv_a):
                if a0 < c1 and a1 > c0 and i not in a_waited:
                    a_waited.add(i)
                    for cp in cps:
                        cp.wait_recv()
            for cb in range(c0, c1):
                scv[0, cb] = (pc[cb, F:HI, :] + rv[1, cb, 0:LO, :].astype(F32)).astype(BF)
                scv[1, cb] = (pc[cb, HI:HI + LO, :] + rv[0, cb, 0:LO, :].astype(F32)).astype(BF)
            sbuf, rbuf = scv, rcv
        else:
            if not mid_waited:
                mid_waited = True
                for pos in range(4):
                    @pl.when(me == pos)
                    def _(pos=pos):
                        mid_copy(pos ^ 1, 0).wait_recv()
                        mid_copy(3 - pos, 1).wait_recv()
            for cb in range(c0, c1):
                for s in range(NS):
                    q = s * NB + cb
                    rs = slice(16 * s, 16 * s + 16)
                    extra = jnp.where(q >= q_p2, rm[1, q].astype(F32), 0.0)
                    scf[0, cb, rs, :] = (pc[cb, rs, :] + extra).astype(BF)
                    extra = jnp.where(q < q_p1, rm[0, q].astype(F32), 0.0)
                    r0 = HI + LO + 16 * s
                    scf[1, cb, rs, :] = (pc[cb, r0:r0 + 16, :] + extra).astype(BF)
            sbuf, rbuf = scf, rcf
        cps = [rdma(sbuf.at[link, pl.ds(c0, c1 - c0)], rbuf.at[link, pl.ds(c0, c1 - c0)], link)
               for link in range(2)]
        for cp in cps:
            cp.start()
        recv_c.append((item, cps))
    assert len(a_waited) == len(recv_a) and mid_waited and next_sem[0] == N_RDMA_SEMS

    for cp in recv_b:
        cp.wait_recv()
    for t in range(NB):
        cs = slice(t * 128, (t + 1) * 128)
        o_ref[0:LO, cs] += rv[0, t, LO:2 * LO, :].astype(F32)
        o_ref[HI:CH, cs] += rv[1, t, LO:2 * LO, :].astype(F32)

    for cp in sends:
        cp.wait_send()
    for pos in range(4):
        @pl.when(me == pos)
        def _(pos=pos):
            for link in range(2):
                mid_copy(pos, link).wait_send()

    for j, ((part, c0, c1), cps) in enumerate(recv_c):
        if j == len(recv_c) - 1:
            for _, cc in recv_c:
                for cp in cc:
                    cp.wait_send()
        for cp in cps:
            cp.wait_recv()
        for t in range(c0, c1):
            cs = slice(t * 128, (t + 1) * 128)
            if part == "V":
                o_ref[0:LO, cs] += rcv[1, t].astype(F32)
                o_ref[HI:CH, cs] += rcv[0, t].astype(F32)
            else:
                o_ref[LO:HI, cs] += rcf[0, t].astype(F32) + rcf[1, t].astype(F32)


def pallas_dist_matmul_mk_i_outk_m1024_n1024_k512_kernel(A: jax.Array, B: jax.Array):
    return pl.pallas_call(
        _body,
        out_shape=jax.ShapeDtypeStruct((CH, N), F32),
        in_specs=[pl.BlockSpec(memory_space=pl.ANY), pl.BlockSpec(memory_space=pl.ANY)],
        out_specs=pl.BlockSpec(memory_space=pltpu.VMEM),
        scratch_shapes=[
            pltpu.VMEM((M, K), F32),
            pltpu.VMEM((NB, K, 128), F32),
            pltpu.VMEM((2, NB, 2 * LO, 128), BF),
            pltpu.VMEM((2, NB, 2 * LO, 128), BF),
            pltpu.VMEM((NQ, 16, 128), BF),
            pltpu.VMEM((2, NQ, 16, 128), BF),
            pltpu.VMEM((2, NB, LO, 128), BF),
            pltpu.VMEM((2, NB, LO, 128), BF),
            pltpu.VMEM((2, NB, F, 128), BF),
            pltpu.VMEM((2, NB, F, 128), BF),
            pltpu.VMEM((NB, 2 * HI, 128), F32),
            pltpu.SemaphoreType.DMA((N_LOAD_SEMS,)),
            pltpu.SemaphoreType.DMA((N_RDMA_SEMS,)),
            pltpu.SemaphoreType.DMA((N_RDMA_SEMS,)),
        ],
        compiler_params=pltpu.CompilerParams(
            collective_id=0,
            vmem_limit_bytes=48 * 1024 * 1024,
            disable_bounds_checks=True,
            disable_semaphore_checks=True,
        ),
    )(A, B)
```

```python
import jax
import jax.numpy as jnp
from jax import lax
from jax.experimental import pallas as pl
from jax.experimental.pallas import tpu as pltpu

M, K, N = 1024, 512, 1024
CH = 256
NB = N // 128
BF = jnp.bfloat16
F32 = jnp.float32

LO = 96
HI = CH - LO
F = HI - LO
NS = F // 16
NQ = NS * NB
_D = 10
Q = (NQ // 2, NQ // 2 - _D, NQ // 2, NQ // 2 + _D)

RG = (0, 16, 48, 80, 96, 128, 160, 192)
MID0 = 4 * LO
C0 = MID0 + F
OWN0 = C0 + 2 * HI

ORDER = ("B0 R0 R1 R2 R3 R4 R5 R6 B1 B2 B3 B4 B5 B6 B7 M C O").split()
PIECES = (
    (0, 1, 0, 1, (0, 1)),
    (1, 2, 0, 1, (1, 2)),
    (2, 3, 0, 1, (2, 3)),
    (3, 5, 0, 1, (3, 5)),
    (5, 6, 0, 1, (5, 6)),
    (6, 7, 0, 1, (6, 7)),
    (0, 4, 1, 2, (0, 1, 2, 4)),
    (4, 7, 1, 2, (4, 7)),
    (0, 4, 2, 3, (0, 4)),
    (0, 4, 3, 4, (0, 4)),
    (0, 4, 4, 6, (0, 4)),
    (0, 4, 6, 8, (0, 4)),
    "M",
    (4, 7, 2, 5, (4, 7)),
    (4, 7, 5, 8, (4, 7)),
)
PC = (("V", 0, 4), ("V", 4, 8), "own", ("F", 0, 6), ("F", 6, 8))

N_LOAD_SEMS = sum(2 if it[0] in "RC" else 1 for it in ORDER)
N_RDMA_SEMS = (2
               + 2 * sum(len(p[4]) - 1 for p in PIECES if p != "M")
               + 2 * sum(1 for p in PC if p != "own"))


def _body(a_hbm, b_hbm, o_ref, a32, b32, sv, rv, sm, rm, scv, rcv, scf, rcf, pc,
          lsem, ssem, rsem):
    me = lax.axis_index("i")
    p1 = me ^ 1
    p2 = 3 - me
    dg = me ^ 2
    nbr = (p1, p2)

    def a_items(item):
        if item[0] == "R":
            g = int(item[1:])
            v0, v1 = RG[g], RG[g + 1]
            n = v1 - v0
            if v0 < LO:
                return [(dg, v0, n, 2 * v0), (dg, HI + v0, n, 2 * v0 + n)]
            return [(p1, v0 - LO, n, 2 * v0), (p2, HI + v0 - LO, n, 2 * v0 + n)]
        if item == "M":
            return [(dg, LO, F, MID0)]
        if item == "C":
            return [(p1, LO, HI, C0), (p2, 0, HI, C0 + HI)]
        return [(me, 0, CH, OWN0)]

    loads = {}
    k = 0
    for item in ORDER:
        cps = []
        if item[0] == "B":
            cb = int(item[1:])
            cps.append(pltpu.make_async_copy(
                b_hbm.at[:, pl.ds(cb * 128, 128)], b32.at[cb], lsem.at[k]))
            k += 1
        else:
            for (c, r0, n, d0) in a_items(item):
                src = pl.multiple_of(c * CH + r0, 16)
                cps.append(pltpu.make_async_copy(
                    a_hbm.at[pl.ds(src, n), :], a32.at[pl.ds(d0, n), :], lsem.at[k]))
                k += 1
        loads[item] = cps

    bar = pltpu.get_barrier_semaphore()
    for i, item in enumerate(ORDER):
        for cp in loads[item]:
            cp.start()
        if i == 0:
            for nb in nbr:
                pl.semaphore_signal(bar, inc=1, device_id=(nb,),
                                    device_id_type=pl.DeviceIdType.MESH)

    def q_of(x):
        r = jnp.int32(Q[0])
        for pos in range(1, 4):
            r = jnp.where(x == pos, jnp.int32(Q[pos]), r)
        return r

    q_p1, q_p2 = q_of(p1), q_of(p2)

    loaded = set()

    def need(items):
        for it in sorted(items, key=ORDER.index):
            if it not in loaded:
                loaded.add(it)
                for cp in loads[it]:
                    cp.wait()

    def lhs(r0, n):
        return a32[pl.ds(r0, n), :].astype(BF)

    def mm(x, cb):
        return jnp.dot(x, b32[cb].astype(BF), preferred_element_type=F32)

    next_sem = [2]

    def rdma(src, dst, link, kk=None):
        if kk is None:
            kk = next_sem[0]
            next_sem[0] += 1
        return pltpu.make_async_remote_copy(
            src_ref=src, dst_ref=dst, send_sem=ssem.at[kk], recv_sem=rsem.at[kk],
            device_id=(nbr[link],), device_id_type=pl.DeviceIdType.MESH)

    def mid_copy(sender_pos, link):
        lo, hi = (0, Q[sender_pos]) if link == 0 else (Q[sender_pos], NQ)
        return rdma(sm.at[pl.ds(lo, hi - lo)], rm.at[link, pl.ds(lo, hi - lo)], link, link)

    sends = []
    recv_a = []
    recv_b = []
    first = True
    for p in PIECES:
        if p == "M":
            need(["M"] + [f"B{c}" for c in range(NB)])
            x = lhs(MID0, F)
            for cb in range(NB):
                res = mm(x, cb).astype(BF)
                for s in range(NS):
                    sm[s * NB + cb] = res[16 * s:16 * s + 16]
            for pos in range(4):
                @pl.when(me == pos)
                def _(pos=pos):
                    for link in range(2):
                        mid_copy(pos, link).start()
            continue
        g0, g1, c0, c1, subs = p
        need([f"R{g}" for g in range(g0, g1)] + [f"B{c}" for c in range(c0, c1)])
        v0, v1 = RG[g0], RG[g1]
        x = lhs(2 * v0, 2 * (v1 - v0))
        ress = [mm(x, cb).astype(BF) for cb in range(c0, c1)]
        for h0, h1 in zip(subs[:-1], subs[1:]):
            for cb in range(c0, c1):
                res = ress[cb - c0]
                for g in range(h0, h1):
                    w0, w1 = RG[g], RG[g + 1]
                    n = w1 - w0
                    off = 2 * (w0 - v0)
                    sv[0, cb, w0:w1, :] = res[off:off + n]
                    sv[1, cb, w0:w1, :] = res[off + n:off + 2 * n]
            u0, u1 = RG[h0], RG[h1]
            cps = [rdma(sv.at[link, pl.ds(c0, c1 - c0), pl.ds(u0, u1 - u0), :],
                        rv.at[link, pl.ds(c0, c1 - c0), pl.ds(u0, u1 - u0), :], link)
                   for link in range(2)]
            if first:
                pl.semaphore_wait(bar, 2)
                first = False
            for cp in cps:
                cp.start()
            sends += cps
            if u0 < LO:
                recv_a.append((c0, c1, cps))
            else:
                recv_b += cps

    need(["C"])
    x = lhs(C0, 2 * HI)
    for cb in range(NB):
        pc[cb] = mm(x, cb)

    a_waited = set()
    mid_waited = False
    recv_c = []
    for item in PC:
        if item == "own":
            need(["O"])
            x = lhs(OWN0, CH)
            for cb in range(NB):
                o_ref[:, cb * 128:(cb + 1) * 128] = mm(x, cb)
            continue
        part, c0, c1 = item
        if part == "V":
            for i, (a0, a1, cps) in enumerate(recv_a):
                if a0 < c1 and a1 > c0 and i not in a_waited:
                    a_waited.add(i)
                    for cp in cps:
                        cp.wait_recv()
            for cb in range(c0, c1):
                scv[0, cb] = (pc[cb, F:HI, :] + rv[1, cb, 0:LO, :].astype(F32)).astype(BF)
                scv[1, cb] = (pc[cb, HI:HI + LO, :] + rv[0, cb, 0:LO, :].astype(F32)).astype(BF)
            sbuf, rbuf = scv, rcv
        else:
            if not mid_waited:
                mid_waited = True
                for pos in range(4):
                    @pl.when(me == pos)
                    def _(pos=pos):
                        mid_copy(pos ^ 1, 0).wait_recv()
                        mid_copy(3 - pos, 1).wait_recv()
            for cb in range(c0, c1):
                for s in range(NS):
                    q = s * NB + cb
                    rs = slice(16 * s, 16 * s + 16)
                    extra = jnp.where(q >= q_p2, rm[1, q].astype(F32), 0.0)
                    scf[0, cb, rs, :] = (pc[cb, rs, :] + extra).astype(BF)
                    extra = jnp.where(q < q_p1, rm[0, q].astype(F32), 0.0)
                    r0 = HI + LO + 16 * s
                    scf[1, cb, rs, :] = (pc[cb, r0:r0 + 16, :] + extra).astype(BF)
            sbuf, rbuf = scf, rcf
        cps = [rdma(sbuf.at[link, pl.ds(c0, c1 - c0)], rbuf.at[link, pl.ds(c0, c1 - c0)], link)
               for link in range(2)]
        for cp in cps:
            cp.start()
        recv_c.append((item, cps))
    assert len(a_waited) == len(recv_a) and mid_waited and next_sem[0] == N_RDMA_SEMS

    for cp in recv_b:
        cp.wait_recv()
    for t in range(NB):
        cs = slice(t * 128, (t + 1) * 128)
        o_ref[0:LO, cs] += rv[0, t, LO:2 * LO, :].astype(F32)
        o_ref[HI:CH, cs] += rv[1, t, LO:2 * LO, :].astype(F32)

    for cp in sends:
        cp.wait_send()
    for pos in range(4):
        @pl.when(me == pos)
        def _(pos=pos):
            for link in range(2):
                mid_copy(pos, link).wait_send()

    for j, ((part, c0, c1), cps) in enumerate(recv_c):
        if j == len(recv_c) - 1:
            for _, cc in recv_c:
                for cp in cc:
                    cp.wait_send()
        for cp in cps:
            cp.wait_recv()
        for t in range(c0, c1):
            cs = slice(t * 128, (t + 1) * 128)
            if part == "V":
                o_ref[0:LO, cs] += rcv[1, t].astype(F32)
                o_ref[HI:CH, cs] += rcv[0, t].astype(F32)
            else:
                o_ref[LO:HI, cs] += rcf[0, t].astype(F32) + rcf[1, t].astype(F32)


def _compiler_params():
    base = dict(collective_id=0, vmem_limit_bytes=48 * 1024 * 1024)
    try:
        return pltpu.CompilerParams(
            disable_bounds_checks=True, disable_semaphore_checks=True, **base)
    except TypeError:
        return pltpu.CompilerParams(**base)


def pallas_dist_matmul_mk_i_outk_m1024_n1024_k512_kernel(A: jax.Array, B: jax.Array):
    return pl.pallas_call(
        _body,
        out_shape=jax.ShapeDtypeStruct((CH, N), F32),
        in_specs=[pl.BlockSpec(memory_space=pl.ANY), pl.BlockSpec(memory_space=pl.ANY)],
        out_specs=pl.BlockSpec(memory_space=pltpu.VMEM),
        scratch_shapes=[
            pltpu.VMEM((M, K), F32),
            pltpu.VMEM((NB, K, 128), F32),
            pltpu.VMEM((2, NB, 2 * LO, 128), BF),
            pltpu.VMEM((2, NB, 2 * LO, 128), BF),
            pltpu.VMEM((NQ, 16, 128), BF),
            pltpu.VMEM((2, NQ, 16, 128), BF),
            pltpu.VMEM((2, NB, LO, 128), BF),
            pltpu.VMEM((2, NB, LO, 128), BF),
            pltpu.VMEM((2, NB, F, 128), BF),
            pltpu.VMEM((2, NB, F, 128), BF),
            pltpu.VMEM((NB, 2 * HI, 128), F32),
            pltpu.SemaphoreType.DMA((N_LOAD_SEMS,)),
            pltpu.SemaphoreType.DMA((N_RDMA_SEMS,)),
            pltpu.SemaphoreType.DMA((N_RDMA_SEMS,)),
        ],
        compiler_params=_compiler_params(),
    )(A, B)
```
